```python
import numpy as np

kernel_name = "dist_rsx_agy_m2048_n1024"

def setup_inputs():
    return {"x": np.random.randn(2, 2048, 2048).astype(np.float32)}

def reference(x: np.ndarray) -> np.ndarray:
    return x.sum(axis=0)
```

```python
import functools
import jax
import jax.numpy as jnp
from jax import lax
from jax.experimental import pallas as pl
from jax.experimental.pallas import tpu as pltpu

MESH = pl.DeviceIdType.MESH
M, N = 2048, 1024


def make(R=32, LA=4, LR=128, nocheck=True):
    n = M // R
    per_load = LR // R
    nl = M // LR

    def body(x_hbm, o, xin, xs, xr, ld_sem, xr_sem, yr_sem, xs_sem, ys_sem):
        mx = lax.axis_index("x")
        my = lax.axis_index("y")
        xpeer = (1 - mx, my)
        ypeer = (mx, 1 - my)
        bar = pltpu.get_barrier_semaphore()
        pl.semaphore_signal(bar, 1, device_id=xpeer, device_id_type=MESH)
        pl.semaphore_signal(bar, 1, device_id=ypeer, device_id_type=MESH)

        def load(j):
            rows = pl.ds(pl.multiple_of(j * LR, LR), LR)
            return pltpu.make_async_copy(x_hbm.at[0, rows], xin.at[rows], ld_sem.at[j])

        def rows_of(c):
            return pl.ds(pl.multiple_of(c * R, R), R)

        own_cols = pl.ds(pl.multiple_of(my * N, N), N)
        oth_cols = pl.ds(pl.multiple_of((1 - my) * N, N), N)

        def xcopy(c):
            return pltpu.make_async_remote_copy(xs.at[rows_of(c)], xr.at[rows_of(c)], xs_sem, xr_sem.at[c], device_id=xpeer, device_id_type=MESH)

        def ycopy(c):
            blk = o.at[rows_of(c), own_cols]
            return pltpu.make_async_remote_copy(blk, blk, ys_sem, yr_sem, device_id=ypeer, device_id_type=MESH)

        for j in range(nl):
            load(j).start()

        def stage_a(c):
            @pl.when(c % per_load == 0)
            def _():
                load(c // per_load).wait()
            xs[rows_of(c), :] = xin[rows_of(c), :].astype(jnp.bfloat16)

        def stage_b(c):
            xcopy(c).wait_recv()
            r = rows_of(c)
            o[r, own_cols] = (xs[r, :].astype(jnp.float32) + xr[r, :].astype(jnp.float32)).astype(jnp.bfloat16)
            ycopy(c).start()

        stage_a(0)
        pl.semaphore_wait(bar, 2)
        xcopy(0).start()

        def pre(c, _):
            stage_a(c)
            xcopy(c).start()
        lax.fori_loop(1, LA, pre, None)

        def step(i, _):
            @pl.when(i + LA < n)
            def _():
                stage_a(i + LA)
                xcopy(i + LA).start()
            stage_b(i)
        lax.fori_loop(0, n, step, None)

        pltpu.make_async_copy(xs, xs, xs_sem).wait()
        pltpu.make_async_copy(xs, xs, ys_sem).wait()
        pltpu.make_async_copy(xs, xs, yr_sem).wait()

    def fn(x):
        return pl.pallas_call(
            body,
            out_shape=jax.ShapeDtypeStruct((M, 2 * N), jnp.bfloat16),
            in_specs=[pl.BlockSpec(memory_space=pltpu.HBM)],
            out_specs=pl.BlockSpec(memory_space=pltpu.VMEM),
            scratch_shapes=[
                pltpu.VMEM((M, N), jnp.float32),
                pltpu.VMEM((M, N), jnp.bfloat16),
                pltpu.VMEM((M, N), jnp.bfloat16),
                pltpu.SemaphoreType.DMA((nl,)),
                pltpu.SemaphoreType.DMA((n,)),
                pltpu.SemaphoreType.DMA,
                pltpu.SemaphoreType.DMA,
                pltpu.SemaphoreType.DMA,
            ],
            compiler_params=pltpu.CompilerParams(
                collective_id=0, vmem_limit_bytes=64 * 2**20,
                disable_semaphore_checks=nocheck, disable_bounds_checks=nocheck),
        )(x)
    return fn


def pallas_dist_rsx_agy_m2048_n1024_kernel(x):
    return make(R=64, LA=2, LR=64)(x)
```

```python
import jax
import jax.numpy as jnp
from jax import lax
from jax.experimental import pallas as pl
from jax.experimental.pallas import tpu as pltpu

M, N = 2048, 1024
HALF = M // 2
LANES = 128
ROWS = 32
CHUNKS = HALF // ROWS
H = ROWS // 2
GROUPS = N // LANES // 2

HEADER = 8
CODE, LOW, SIGN = 0, H, (1 + GROUPS) * H
MSG = SIGN + H // 2
END = HEADER + CHUNKS * MSG + H

AHEAD = 3
LAG_Y, LAG_D = 3, 2
REROUTED = 136

SCATTER_OUT, OWN, SCATTER_IN, FROM_X, FROM_Y, FROM_D = range(6)

I32 = jnp.int32
BYTE_ONE = 0x01010101
BYTE_TOP = 0x80808080 - (1 << 32)


def _shl(x, n):
    return lax.shift_left(x, n if isinstance(n, jax.Array) else jnp.full_like(x, n))


def _shr(x, n):
    return lax.shift_right_logical(x, n if isinstance(n, jax.Array) else jnp.full_like(x, n))


def _swap_bytes(a, b):
    t = (_shr(a, 8) ^ b) & 0x00FF00FF
    return a ^ _shl(t, 8), b ^ t


def _pick_origin(words):
    magnitude = (_shr(words, 16) & 0x7FFF).astype(jnp.float32)
    total = jnp.sum(jnp.sum(magnitude, axis=0, keepdims=True), axis=1, keepdims=True)
    origin = (total * (1.0 / magnitude.size) + 220.0).astype(I32) & 0xFFFF
    return jnp.broadcast_to(origin * 0x00010001, words.shape)


def _encode(high, queue, fill):
    bad = spill = None
    for g, byte in enumerate(high):
        e = byte & 0x7F7F7F7F
        e1 = e + BYTE_ONE
        above = e1 & BYTE_TOP
        lengths = (e1 ^ above) + _shr((e + 0x7E7E7E7E) & BYTE_TOP, 7) + _shr(above, 6)
        total = _shr(lengths * BYTE_ONE, 24)
        check = (lengths & (0xE0E0E0E0 - (1 << 32))) | (total & ~31)
        bad = check if g == 0 else bad | check
        code = _shl(jnp.ones_like(e), _shr(lengths, 8) & 0xFF) | 1
        code = _shl(code, _shr(lengths, 16) & 0xFF) | 1
        code = _shl(code, _shr(lengths, 24)) | 1
        out = _shr(queue, 32 - total)
        spill = out if g == 0 else _shl(spill, total) | out
        queue = _shl(queue, total) | code
        fill = fill + total
    extra = fill - 32
    fill = jnp.where(extra < 0, 0, extra)
    word = _shr(_shl(queue, fill - extra), fill) | _shl(_shl(spill, 1), 31 - fill)
    return word, queue, fill, bad | (fill & ~31)


def _decode(signs, head, tail, fill):
    high = []
    top = jnp.full_like(head, -(1 << 31))
    for g in range(GROUPS):
        p0 = lax.clz(head)
        x = head ^ _shr(top, p0)
        p1 = lax.clz(x)
        x = x ^ _shr(top, p1)
        p2 = lax.clz(x)
        x = x ^ _shr(top, p2)
        p3 = lax.clz(x)
        ends = p0 | _shl(p1, 8) | _shl(p2, 16) | _shl(p3, 24)
        zeros = ends * (1 - 256) - 0x01010100
        if g < GROUPS - 1:
            head = _shl(head, p3 + 1) | _shr(tail, 31 - p3)
            tail = _shl(tail, p3 + 1)
        fill = fill + p3
        ge2 = (zeros + 0x7E7E7E7E) & BYTE_TOP
        ge3 = (zeros + 0x7D7D7D7D) & BYTE_TOP
        e = zeros - _shr(ge2, 7) + _shr(ge2 ^ ge3, 7) * 126
        high.append(e | (_shl(signs, GROUPS - 1 - g) & BYTE_TOP))
    fill = fill + (GROUPS - 32)
    return high, jnp.where(fill < 0, 0, fill)


def _body(x_hbm, out, xin, msg, raw, state, highs, raw_sends,
          load_sem, recv_sem, late_sem, raw_sem, edge_sem, send_sem, raw_send_sem, hello_sem):
    mx = lax.axis_index("x")
    my = lax.axis_index("y")
    xpeer = (1 - mx, my)
    ypeer = (mx, 1 - my)

    def signal(sem, peer):
        pl.semaphore_signal(sem, 1, device_id=peer, device_id_type=pl.DeviceIdType.MESH)

    is_00 = jnp.logical_and(mx == 0, my == 0)
    is_01 = jnp.logical_and(mx == 0, my == 1)
    barrier = pltpu.get_barrier_semaphore()
    signal(barrier, xpeer)
    pl.when(is_01)(lambda: signal(barrier, ypeer))

    load_rows = (32, 32, 64, 128, 256, 512)
    load_start = [sum(load_rows[:j]) for j in range(len(load_rows))]

    def load(half, j):
        first = pl.multiple_of((mx if half else 1 - mx) * HALF + load_start[j], ROWS)
        return pltpu.make_async_copy(
            x_hbm.at[0, pl.ds(first, load_rows[j])],
            xin.at[half, pl.ds(load_start[j], load_rows[j])],
            load_sem.at[half * len(load_rows) + j])

    def wait_load(half, c):
        for j, first in enumerate(load_start):
            if isinstance(c, int):
                if c * ROWS == first:
                    load(half, j).wait()
            elif first > ROWS * (1 - half):
                pl.when(c * ROWS == first)(lambda: load(half, j).wait())

    for half, j in [(0, 0), (0, 1), (0, 2), (1, 0), (1, 1), (1, 2)]:
        load(half, j).start()
    for j in range(3, len(load_rows)):
        load(0, j).start()
        load(1, j).start()

    state[...] = jnp.zeros_like(state)
    raw_sends[0] = 0

    def slot(c, offset, size=H):
        return pl.ds(pl.multiple_of(HEADER + c * MSG + offset, 8), size)

    def raw_slot(c, g, size=H):
        return pl.ds(pl.multiple_of((c * GROUPS + g) * H, H), size)

    def remote(src, dst, ssem, rsem, peer):
        return pltpu.make_async_remote_copy(
            src, dst, ssem, rsem, device_id=peer, device_id_type=pl.DeviceIdType.MESH)

    def send(src, dst, rows, sem, peer):
        return remote(msg.at[src, rows], msg.at[dst, rows], send_sem, sem, peer)

    def sem(dst, c):
        return recv_sem.at[(dst - SCATTER_IN) * CHUNKS + c]

    def send_raw(src, dst, c, peer):
        rows = raw_slot(c, 0, GROUPS * H)
        return remote(raw.at[src, rows], raw.at[dst, rows], raw_send_sem,
                      raw_sem.at[(dst - SCATTER_IN) * CHUNKS + c], peer)

    def completing(c, fn):
        pl.when(c == 0)(lambda: fn(pl.ds(HEADER - 1, 1 + H + MSG)))
        pl.when(c > 0)(lambda: fn(slot(c, H, MSG)))

    def origin_of(s):
        return jnp.broadcast_to(msg[s, pl.ds(HEADER - 1, 1), :], (H, LANES))

    def pack_low(s, c, g, a, b, origin):
        low, high = _swap_bytes(origin - a, origin - b)
        msg[s, slot(c, LOW + g * H), :] = low
        return high

    def pack_signs(s, c, high):
        signs = high[0] & BYTE_TOP
        for byte in high[1:]:
            signs = _shr(signs, 1) | (byte & BYTE_TOP)
        msg[s, slot(c, SIGN, H // 2), :] = signs[:H // 2] | _shr(signs[H // 2:], 4)

    def pack_high(s, c, high, targets):
        queue, fill = state[s, 0], state[s, 1]
        word, new_queue, new_fill, bad = _encode(high, queue, fill)
        msg[s, slot(c, CODE), :] = word
        state[s, 0] = new_queue
        state[s, 1] = new_fill

        @pl.when(jnp.max(jnp.where(bad != 0, 1.0, 0.0)) > 0.0)
        def _():
            msg[s, slot(c, CODE), :] = _shl(_shl(queue, 1), 31 - fill)
            state[s, 0] = jnp.zeros_like(queue)
            state[s, 1] = fill
            for g in range(GROUPS):
                raw[s, raw_slot(c, g), :] = high[g]
            for dst, peer in targets:
                send_raw(s, dst, c, peer).start()
            raw_sends[0] = raw_sends[0] + len(targets)

    def flush(s):
        msg[s, slot(CHUNKS, CODE), :] = _shl(_shl(state[s, 0], 1), 31 - state[s, 1])

    def unpack_high(s, c, relay_raw=None):
        fill = state[s, 1]
        word, next_word = msg[s, slot(c, CODE), :], msg[s, slot(c + 1, CODE), :]
        head = _shl(word, fill) | _shr(_shr(next_word, 1), 31 - fill)
        signs = msg[s, slot(c, SIGN, H // 2), :]
        signs = jnp.concatenate([signs, _shl(signs, 4)], axis=0)
        high, new_fill = _decode(signs, head, _shl(next_word, fill), fill)
        state[s, 1] = jnp.where(head == 0, fill, new_fill)
        for g in range(GROUPS):
            highs[g] = high[g]

        @pl.when(head[0, 0] == 0)
        def _():
            send_raw(s, s, c, xpeer).wait_recv()
            if relay_raw is not None:
                relay_raw()
            for g in range(GROUPS):
                highs[g] = raw[s, raw_slot(c, g), :]

    def unpack_low(s, c, g, origin):
        a, b = _swap_bytes(msg[s, slot(c, LOW + g * H), :], highs[g])
        return pltpu.bitcast(origin - a, jnp.bfloat16), pltpu.bitcast(origin - b, jnp.bfloat16)

    def tile(half, c, k):
        return xin[half, pl.ds(pl.multiple_of(c * ROWS, ROWS), ROWS), pl.ds(k * LANES, LANES)]

    def put(qx, qy, c, k, value):
        out[pl.ds(pl.multiple_of(qx * HALF + c * ROWS, ROWS), ROWS),
            pl.ds(pl.multiple_of(qy * N + k * LANES, LANES), LANES)] = value

    def scatter_low(c, first=False):
        words = [pltpu.bitcast(tile(0, c, k).astype(jnp.bfloat16), I32) for k in range(2 * GROUPS)]
        if first:
            origin = _pick_origin(words[0])
            msg[SCATTER_OUT, pl.ds(0, HEADER), :] = origin[:HEADER]
        else:
            origin = origin_of(SCATTER_OUT)
        high = [pack_low(SCATTER_OUT, c, g, words[2 * g], words[2 * g + 1], origin)
                for g in range(GROUPS)]
        pack_signs(SCATTER_OUT, c, high)
        return high

    def scatter_early(c):
        return send(SCATTER_OUT, SCATTER_IN, slot(c, LOW + 2 * H, MSG - 2 * H), sem(SCATTER_IN, c), xpeer)

    def scatter_late(c):
        return send(SCATTER_OUT, SCATTER_IN, slot(c, LOW, 2 * H), late_sem.at[c], xpeer)

    def scatter(c):
        wait_load(0, c)
        pack_high(SCATTER_OUT, c, scatter_low(c), [(SCATTER_IN, xpeer)])
        scatter_early(c - 1).start()
        scatter_late(c - 1).start()

    def reduce(c, first=False):
        unpack_high(SCATTER_IN, c)
        origin_in = origin_of(SCATTER_IN)
        origin = None if first else origin_of(OWN)
        high = {}
        for g in (2, 3, 0, 1):
            if g == 0:
                send(OWN, FROM_Y, slot(c, LOW + 2 * H, 2 * H), sem(FROM_Y, c), ypeer).start()
                scatter_late(c).wait_recv()
            sums = []
            for k, theirs in zip((2 * g, 2 * g + 1), unpack_low(SCATTER_IN, c, g, origin_in)):
                total = (tile(1, c, k) + theirs.astype(jnp.float32)).astype(jnp.bfloat16)
                put(mx, my, c, k, total)
                sums.append(pltpu.bitcast(total, I32))
            if origin is None:
                origin = _pick_origin(sums[0])
                msg[OWN, pl.ds(0, HEADER), :] = origin[:HEADER]
            high[g] = pack_low(OWN, c, g, *sums, origin)
        high = [high[g] for g in range(GROUPS)]
        pack_signs(OWN, c, high)
        send(OWN, FROM_Y, slot(c, SIGN, H // 2), sem(FROM_Y, c), ypeer).start()
        pack_high(OWN, c, high, [(FROM_Y, ypeer), (FROM_X, xpeer)])
        rows = pl.ds(HEADER - 1, 1 + 3 * H) if first else slot(c, CODE, 3 * H)
        send(OWN, FROM_Y, rows, sem(FROM_Y, c), ypeer).start()

    def gather(s, c):
        def relay_raw():
            @pl.when(s == FROM_X)
            def _():
                send_raw(s, FROM_D, c, ypeer).start()
                raw_sends[0] = raw_sends[0] + 1

        unpack_high(s, c, relay_raw)
        qx = jnp.where(s == FROM_Y, mx, 1 - mx)
        qy = jnp.where(s == FROM_X, my, 1 - my)
        origin = origin_of(s)
        for g in range(GROUPS):
            for k, value in zip((2 * g, 2 * g + 1), unpack_low(s, c, g, origin)):
                put(qx, qy, c, k, value)

    def wait_y(c):
        if isinstance(c, int):
            rows = pl.ds(HEADER - 1, 1 + MSG) if c == 0 else slot(c, CODE, MSG + H * (c == CHUNKS - 1))
            send(FROM_Y, FROM_Y, rows, sem(FROM_Y, c), ypeer).wait_recv()
        else:
            pl.when(c == 0)(lambda: wait_y(0))
            pl.when(c > 0)(
                lambda: send(FROM_Y, FROM_Y, slot(c, CODE, MSG), sem(FROM_Y, c), ypeer).wait_recv())

    last = CHUNKS - 1
    via_y = pl.ds(END - 2 * MSG, 2 * MSG - REROUTED)
    via_x = [(pl.ds(END - REROUTED, REROUTED - MSG), edge_sem.at[2]),
             (pl.ds(END - MSG, MSG), sem(FROM_D, last))]

    def wait_d(c):
        pl.when(c < last - 1)(lambda: completing(
            c, lambda rows: send(FROM_D, FROM_D, rows, sem(FROM_D, c), ypeer).wait_recv()))

        @pl.when(c == last - 1)
        def _():
            send(FROM_D, FROM_D, via_y, sem(FROM_D, last - 1), ypeer).wait_recv()
            send(FROM_D, FROM_D, *via_x[0], xpeer).wait_recv()

        pl.when(c == last)(lambda: send(FROM_D, FROM_D, *via_x[1], xpeer).wait_recv())

    def step(i, _):
        @pl.when(i <= last)
        def _():
            wait_load(1, i)
            scatter_early(i).wait_recv()
            reduce(i)
            completing(i - 1, lambda rows: send(OWN, FROM_X, rows, sem(FROM_X, i - 1), xpeer).start())

            @pl.when(i == last)
            def _():
                flush(OWN)
                send(OWN, FROM_Y, slot(CHUNKS, CODE), sem(FROM_Y, last), ypeer).start()
                send(OWN, FROM_X, slot(last, H, MSG), sem(FROM_X, last), xpeer).start()

        pl.when(i + AHEAD < last)(lambda: scatter(i + AHEAD + 1))

        @pl.when(i + AHEAD == last)
        def _():
            flush(SCATTER_OUT)
            scatter_early(last).start()
            scatter_late(last).start()

        f = i - AHEAD

        @pl.when(f >= 0)
        def _():
            def relay(rows):
                send(FROM_X, FROM_X, rows, sem(FROM_X, f), xpeer).wait_recv()
                pl.when(f < last - 1)(
                    lambda: send(FROM_X, FROM_D, rows, sem(FROM_D, f), ypeer).start())

            completing(f, relay)
            pl.when(f == last - 1)(
                lambda: send(FROM_X, FROM_D, via_y, sem(FROM_D, last - 1), ypeer).start())

        g = i - LAG_Y + 1
        pl.when(jnp.logical_and(g >= 0, i <= CHUNKS))(lambda: wait_y(g))

        def decode_one(j, _):
            s = FROM_X + jnp.minimum(j, 2)
            c = jnp.where(j == 0, f, jnp.where(j == 1, i - LAG_Y, f - LAG_D + j - 2))

            @pl.when(c >= 0)
            def _():
                pl.when(s == FROM_D)(lambda: wait_d(c))
                gather(s, c)

        lax.fori_loop(0, jnp.where(f == last, 3 + LAG_D, 3), decode_one, None)

        @pl.when(i == CHUNKS)
        def _():
            for c in range(CHUNKS - LAG_Y + 2, CHUNKS):
                wait_y(c)
            for rows, arrived in via_x:
                send(FROM_Y, FROM_D, rows, arrived, xpeer).start()

    first_parts = [
        send(SCATTER_OUT, SCATTER_IN, slot(0, LOW + 2 * H, 2 * H + H // 2), sem(SCATTER_IN, 0), xpeer),
        send(SCATTER_OUT, SCATTER_IN, pl.ds(HEADER - 1, 1 + H), edge_sem.at[0], xpeer),
        send(SCATTER_OUT, SCATTER_IN, slot(1, CODE), edge_sem.at[1], xpeer),
    ]
    wait_load(0, 0)
    high = scatter_low(0, first=True)
    pl.when(is_00)(lambda: pl.semaphore_wait(barrier, 2))
    pl.when(jnp.logical_not(is_00))(lambda: pl.semaphore_wait(barrier, 1))
    first_parts[0].start()
    pl.when(is_00)(lambda: signal(hello_sem, ypeer))
    pack_high(SCATTER_OUT, 0, high, [(SCATTER_IN, xpeer)])
    first_parts[1].start()

    @pl.when(is_01)
    def _():
        pl.semaphore_wait(hello_sem, 1)
        signal(hello_sem, xpeer)
        signal(hello_sem, ypeer)

    wait_load(0, 1)
    pack_high(SCATTER_OUT, 1, scatter_low(1), [(SCATTER_IN, xpeer)])
    first_parts[2].start()
    scatter_late(0).start()
    lax.fori_loop(2, AHEAD + 1, lambda c, _: scatter(c), None)
    pl.when(jnp.logical_not(is_01))(lambda: pl.semaphore_wait(hello_sem, 1))
    pl.when(is_00)(lambda: signal(hello_sem, xpeer))

    wait_load(1, 0)
    for part in first_parts:
        part.wait_recv()
    reduce(0, first=True)
    scatter(AHEAD + 1)
    lax.fori_loop(1, CHUNKS + AHEAD, step, None)

    sent = msg.at[pl.ds(0, 4), pl.ds(HEADER - 1, END - HEADER + 1)]
    pltpu.make_async_copy(sent, sent, send_sem).wait()
    lax.fori_loop(
        0, raw_sends[0], lambda j, _: send_raw(SCATTER_OUT, SCATTER_IN, 0, xpeer).wait_send(), None)


def pallas_dist_rsx_agy_m2048_n1024_kernel(x: jax.Array):
    dma = pltpu.SemaphoreType.DMA
    return pl.pallas_call(
        _body,
        out_shape=jax.ShapeDtypeStruct((M, 2 * N), jnp.bfloat16),
        in_specs=[pl.BlockSpec(memory_space=pltpu.HBM)],
        out_specs=pl.BlockSpec(memory_space=pltpu.VMEM),
        scratch_shapes=[
            pltpu.VMEM((2, HALF, N), jnp.float32),
            pltpu.VMEM((6, END, LANES), I32),
            pltpu.VMEM((6, CHUNKS * GROUPS * H, LANES), I32),
            pltpu.VMEM((6, 2, H, LANES), I32),
            pltpu.VMEM((GROUPS, H, LANES), I32),
            pltpu.SMEM((1,), I32),
            dma((12,)),
            dma((4 * CHUNKS,)),
            dma((CHUNKS,)),
            dma((4 * CHUNKS,)),
            dma((3,)),
            dma,
            dma,
            pltpu.SemaphoreType.REGULAR,
        ],
        compiler_params=pltpu.CompilerParams(
            collective_id=0,
            vmem_limit_bytes=64 * 2**20,
            disable_semaphore_checks=True,
        ),
        name="rsx_agy",
    )(x)
```

```python
import jax
import jax.numpy as jnp
from jax import lax
from jax.experimental import pallas as pl
from jax.experimental.pallas import tpu as pltpu

M, N = 2048, 1024
HALF = M // 2
LANES = 128
ROWS = 32
CHUNKS = HALF // ROWS
LAST = CHUNKS - 1
H = ROWS // 2
GROUPS = N // LANES // 2
RATE = 30
PENDING = 58

ORIGIN = 7
BASE = 8 + 2 * H
SIGN = GROUPS * H
CODE = SIGN + H // 2
STRIDE = CODE + H
SCATTER_OUT, OWN, SCATTER_IN, FROM_X, FROM_Y, FROM_D = range(6)

AHEAD = 3
TAIL = 3
VIA_Y = 52

I32 = jnp.int32
BYTE_ONE = 0x01010101
BYTE_TOP = 0x80808080 - (1 << 32)


def _shl(x, n):
    return lax.shift_left(x, n if isinstance(n, jax.Array) else jnp.full_like(x, n))


def _shr(x, n):
    return lax.shift_right_logical(x, n if isinstance(n, jax.Array) else jnp.full_like(x, n))


def _funnel(a, b, n):
    return _shl(a, n) | _shr(_shr(b, 1), 31 - n)


def _window(a, b, c, n):
    far = n >= 32
    a, b, c = jnp.where(far, b, a), jnp.where(far, c, b), jnp.where(far, 0, c)
    return _funnel(a, b, n & 31), _funnel(b, c, n & 31)


def _swap_bytes(a, b):
    t = (_shr(a, 8) ^ b) & 0x00FF00FF
    return a ^ _shl(t, 8), b ^ t


def _pick_origin(words):
    magnitude = (_shr(words, 16) & 0x7FFF).astype(jnp.float32)
    total = jnp.sum(jnp.sum(magnitude, axis=0, keepdims=True), axis=1, keepdims=True)
    origin = (total * (1.0 / magnitude.size) + 225.0).astype(I32) & 0xFFFF
    return jnp.broadcast_to(origin * 0x00010001, words.shape)


def _take(q2, q1, q0, fill):
    far = fill >= 32
    upper, lower, n = jnp.where(far, q2, q1), jnp.where(far, q1, q0), fill & 31
    return _shl(_shr(lower, n) | _shl(_shl(upper, 1), 31 - n), 32 - RATE)


def _encode(high, q1, q0, fill):
    bad = q2 = length = None
    for g, byte in enumerate(high):
        e = byte & 0x7F7F7F7F
        e1 = e + BYTE_ONE
        above = e1 & BYTE_TOP
        lengths = (e1 ^ above) + _shr((e + 0x7E7E7E7E) & BYTE_TOP, 7) + _shr(above, 6)
        total = _shr(lengths * BYTE_ONE, 24)
        check = (lengths & (0xE0E0E0E0 - (1 << 32))) | (total & ~31)
        code = _shl(jnp.ones_like(e), _shr(lengths, 8) & 0xFF) | 1
        code = _shl(code, _shr(lengths, 16) & 0xFF) | 1
        code = _shl(code, _shr(lengths, 24)) | 1
        spill = _shr(q1, 32 - total)
        q2 = spill if g == 0 else _shl(q2, total) | spill
        q1 = _shl(q1, total) | _shr(q0, 32 - total)
        q0 = _shl(q0, total) | code
        bad = check if g == 0 else bad | check
        length = total if g == 0 else length + total
    extra = fill + length - RATE
    fill = jnp.where(extra < 0, 0, extra)
    word = _take(q2, q1, _shl(q0, fill - extra), fill)
    bad = bad | _shr(2 * RATE - length, 31)
    bad = bad[:H // 2] | bad[H // 2:] | _shr(PENDING - fill[:H // 2] - fill[H // 2:], 31)
    return word, q1, q0, fill, bad


def _decode(signs, head, tail, fill):
    high = []
    top = jnp.full_like(head, -(1 << 31))
    for g in range(GROUPS):
        p0 = lax.clz(head)
        x = head ^ _shr(top, p0)
        p1 = lax.clz(x)
        x = x ^ _shr(top, p1)
        p2 = lax.clz(x)
        x = x ^ _shr(top, p2)
        p3 = lax.clz(x)
        ends = p0 | _shl(p1, 8) | _shl(p2, 16) | _shl(p3, 24)
        zeros = ends * (1 - 256) - 0x01010100
        if g < GROUPS - 1:
            head = _shl(head, p3 + 1) | _shr(tail, 31 - p3)
            tail = _shl(tail, p3 + 1)
        fill = fill + p3
        ge2 = (zeros + 0x7E7E7E7E) & BYTE_TOP
        ge3 = (zeros + 0x7D7D7D7D) & BYTE_TOP
        e = zeros - _shr(ge2, 7) + _shr(ge2 ^ ge3, 7) * 126
        high.append(e | (_shl(signs, GROUPS - 1 - g) & BYTE_TOP))
    fill = fill + (GROUPS - RATE)
    return high, jnp.where(fill < 0, 0, fill)


def _fold_rows(word):
    row = lax.broadcasted_iota(I32, word.shape, 0)
    last = jnp.broadcast_to(_shr(word[H - 1:], 2), word.shape)
    return word | (_shr(last, 2 * row) & 3)


def _unfold_rows(folded):
    row = lax.broadcasted_iota(I32, folded.shape, 0)
    folded = jnp.where(row < H - 1, folded, 0)
    last = jnp.sum(_shl(folded & 3, 2 * row), axis=0, keepdims=True)
    return jnp.where(row < H - 1, folded & ~3, jnp.broadcast_to(_shl(last, 2), folded.shape))


def _join_pending(q1, q0, fill):
    zero = jnp.zeros_like(fill)
    hi, lo = _window(_shl(q1, 1) | _shr(q0, 31), _shl(q0, 1), zero, 63 - fill)
    n, zero = fill[:H // 2], zero[:H // 2]
    first = _window(zero, hi[:H // 2], lo[:H // 2], zero + 26)
    far = n > 26
    second = _window(zero, jnp.where(far, 0, hi[H // 2:]), jnp.where(far, hi[H // 2:], lo[H // 2:]),
                     jnp.where(far, 58 - n, 26 - n))
    return jnp.concatenate([_shl(n, 26) | first[0] | second[0], first[1] | second[1]], axis=0)


def _split_pending(joined):
    hi, lo = joined[:H // 2], joined[H // 2:]
    zero = jnp.zeros_like(hi)
    first = _window(hi, lo, zero, zero + 6)
    second = _window(*first, zero, _shr(hi, 26))
    hi, lo = (jnp.concatenate(pair, axis=0) for pair in zip(first, second))
    return hi & ~3, _funnel(hi, lo, RATE) & ~3


def _body(x_hbm, out, xin, msg, raw, state, highs, raw_sends,
          load_sem, recv_sem, late_sem, raw_sem, edge_sem, send_sem, raw_send_sem, hello_sem):
    mx = lax.axis_index("x")
    my = lax.axis_index("y")
    xpeer = (1 - mx, my)
    ypeer = (mx, 1 - my)

    def notify(sem, peer):
        pl.semaphore_signal(sem, 1, device_id=peer, device_id_type=pl.DeviceIdType.MESH)

    is_00 = jnp.logical_and(mx == 0, my == 0)
    is_01 = jnp.logical_and(mx == 0, my == 1)
    barrier = pltpu.get_barrier_semaphore()
    notify(barrier, xpeer)
    pl.when(is_01)(lambda: notify(barrier, ypeer))

    load_start = (0, 32, 64, 128, 256, 512, HALF)
    loads = len(load_start) - 1

    def load(half, j, cols=pl.ds(0, N), sem=None):
        size = load_start[j + 1] - load_start[j]
        first = pl.multiple_of((mx if half else 1 - mx) * HALF + load_start[j], ROWS)
        return pltpu.make_async_copy(
            x_hbm.at[0, pl.ds(first, size), cols], xin.at[half, pl.ds(load_start[j], size), cols],
            load_sem.at[half * loads + j if sem is None else sem])

    def wait_load(half, c, js):
        for j in js:
            pl.when(c * ROWS == load_start[j])(lambda: load(half, j).wait())

    first_tiles = load(0, 0, pl.ds(0, 2 * LANES))
    other_tiles = load(0, 0, pl.ds(2 * LANES, N - 2 * LANES), 2 * loads)
    first_tiles.start()
    other_tiles.start()
    for half, j in [(0, 1), (0, 2), (0, 3), (1, 0), (1, 1), (1, 2), (0, 4), (1, 3), (0, 5), (1, 4), (1, 5)]:
        load(half, j).start()

    state[...] = jnp.zeros_like(state)
    raw_sends[0] = 0

    def rows(c, offset, size):
        return pl.ds(pl.multiple_of(BASE + c * STRIDE + offset, 8), size)

    def code_rows(c, size):
        if isinstance(c, int):
            return pl.ds(BASE + (c - 2) * H, size) if c < 2 else rows(c - 2, CODE, size)
        first = jnp.where(c < 2, BASE + (c - 2) * H, BASE + (c - 2) * STRIDE + CODE)
        return pl.ds(pl.multiple_of(first, 8), size)

    def chunk_rows(c, skip=0):
        if c == 0:
            return pl.ds(ORIGIN, BASE - ORIGIN + STRIDE - 1)
        return rows(c, skip, {LAST: CODE, LAST - 1: STRIDE}.get(c, STRIDE - 1) - skip)

    def inner_chunk(c, fn):
        pl.when(c == 0)(lambda: fn(chunk_rows(0)))
        pl.when(jnp.logical_and(c > 0, c < LAST - 1))(lambda: fn(rows(c, 0, STRIDE - 1)))

    def halves(part):
        return pl.ds(part.start, 48), pl.ds(part.start + 48, part.size - 48)

    def raw_rows(c, g, size=H):
        return pl.ds(pl.multiple_of((c * GROUPS + g) * H, H), size)

    def remote(src, dst, sent, arrived, peer):
        return pltpu.make_async_remote_copy(
            src, dst, sent, arrived, device_id=peer, device_id_type=pl.DeviceIdType.MESH)

    def send(src, dst, part, arrived, peer, dst_part=None):
        dst_part = part if dst_part is None else dst_part
        return remote(msg.at[src, part], msg.at[dst, dst_part], send_sem, arrived, peer)

    def wait(s, part, arrived):
        send(s, s, part, arrived, xpeer).wait_recv()

    def sem(s, c):
        return recv_sem.at[(s - SCATTER_IN) * CHUNKS + c]

    def send_raw(src, dst, c, peer):
        part = raw_rows(c, 0, GROUPS * H)
        return remote(raw.at[src, part], raw.at[dst, part], raw_send_sem,
                      raw_sem.at[(dst - SCATTER_IN) * CHUNKS + c], peer)

    def origin_of(s):
        header = msg[s, pl.ds(pl.multiple_of(jnp.where(s == FROM_Y, BASE - 8, 0), 8), 8), :]
        return jnp.broadcast_to(header[7:], (H, LANES))

    def pack_low(s, c, place, a, b, origin):
        low, high = _swap_bytes(origin - a, origin - b)
        msg[s, rows(c, place * H, H), :] = low
        return high

    def pack_signs(s, c, high):
        signs = high[0] & BYTE_TOP
        for byte in high[1:]:
            signs = _shr(signs, 1) | (byte & BYTE_TOP)
        msg[s, rows(c, SIGN, H // 2), :] = signs[:H // 2] | _shr(signs[H // 2:], 4)

    def pack_high(s, c, high, targets):
        q1, q0, fill = state[s, 0], state[s, 1], state[s, 2]
        word, state[s, 0], state[s, 1], state[s, 2], bad = _encode(high, q1, q0, fill)
        msg[s, code_rows(c, H), :] = _fold_rows(word)

        @pl.when(jnp.max(jnp.where(bad != 0, 1.0, 0.0)) > 0.0)
        def _():
            r1, r0 = _shl(q1, RATE) | _shr(q0, 32 - RATE), _shl(q0, RATE)
            msg[s, code_rows(c, H), :] = _fold_rows(_take(_shr(q1, 32 - RATE), r1, r0, fill))
            state[s, 0], state[s, 1], state[s, 2] = r1, r0, fill
            for g in range(GROUPS):
                raw[s, raw_rows(c, g), :] = high[g]
            for dst, peer in targets:
                send_raw(s, dst, c, peer).start()
            raw_sends[0] = raw_sends[0] + len(targets)

    def flush(s):
        msg[s, code_rows(CHUNKS, H), :] = _join_pending(state[s, 0], state[s, 1], state[s, 2])

    def unpack_high(s, c, keep=0, first=False):
        if first:
            w0, w1 = (_unfold_rows(msg[s, code_rows(k, H), :]) for k in range(2))
            w2 = fill = jnp.zeros_like(w0)
        else:
            prompt = s == FROM_Y

            @pl.when(c == 0)
            def _():
                for k in range(2):
                    start = jnp.where(prompt, BASE + k * STRIDE + CODE, BASE + (k - 2) * H)
                    state[s, k] = _unfold_rows(msg[s, pl.ds(pl.multiple_of(start, 8), H), :])

            folded = msg[s, rows(jnp.minimum(c, LAST - 1) + jnp.where(prompt, 2, 0), CODE, H), :]

            @pl.when(c >= LAST - 1)
            def _():
                before_last, last = _split_pending(folded)
                state[s, 3] = jnp.where(c == LAST, last, before_last)

            w0, w1, fill = state[s, 0], state[s, 1], state[s, 2]
            w2 = jnp.where(c < LAST - 1, _unfold_rows(folded), state[s, 3])
        head, tail = _window(w0 | _shr(w1, RATE), _shl(w1, 2) | _shr(w2, RATE - 2), _shl(w2, 4), fill)
        signs = msg[s, rows(c, SIGN, H // 2), :]
        signs = jnp.concatenate([signs, _shl(signs, 4)], axis=0)
        high, new_fill = _decode(signs, head, tail, fill)
        marker = _shr(head, 32 - RATE)
        state[s, 0], state[s, 1], state[s, 2] = w1, w2, jnp.where(marker == 0, fill, new_fill)
        for g in range(GROUPS):
            highs[keep, g] = high[g]

        @pl.when(marker[0, 0] == 0)
        def _():
            send_raw(s, s, c, xpeer).wait_recv()

            @pl.when(s == FROM_X)
            def _():
                send_raw(s, FROM_D, c, ypeer).start()
                raw_sends[0] = raw_sends[0] + 1

            for g in range(GROUPS):
                highs[keep, g] = raw[s, raw_rows(c, g), :]

    def unpack_low(s, c, g, place, origin, keep=0):
        a, b = _swap_bytes(msg[s, rows(c, place * H, H), :], highs[keep, g])
        return pltpu.bitcast(origin - a, jnp.bfloat16), pltpu.bitcast(origin - b, jnp.bfloat16)

    def tile(half, c, k):
        return xin[half, pl.ds(pl.multiple_of(c * ROWS, ROWS), ROWS), pl.ds(k * LANES, LANES)]

    def put(qx, qy, c, k, value):
        out[pl.ds(pl.multiple_of(qx * HALF + c * ROWS, ROWS), ROWS),
            pl.ds(pl.multiple_of(qy * N + k * LANES, LANES), LANES)] = value

    def scatter_group(c, g, origin):
        words = [pltpu.bitcast(tile(0, c, k).astype(jnp.bfloat16), I32) for k in (2 * g, 2 * g + 1)]
        if origin is None:
            origin = _pick_origin(words[0])
            msg[SCATTER_OUT, pl.ds(0, 8), :] = origin[:8]
        return pack_low(SCATTER_OUT, c, g ^ 2, *words, origin), origin

    def scatter_pack(c):
        origin = origin_of(SCATTER_OUT)
        high = [scatter_group(c, g, origin)[0] for g in range(GROUPS)]
        pack_signs(SCATTER_OUT, c, high)
        pack_high(SCATTER_OUT, c, high, [(SCATTER_IN, xpeer)])

    def scatter_send(c, early):
        send(SCATTER_OUT, SCATTER_IN, early, sem(SCATTER_IN, c), xpeer).start()
        send(SCATTER_OUT, SCATTER_IN, rows(c, 0, 2 * H), late_sem.at[c], xpeer).start()

    def scatter(c, _=None):
        wait_load(0, c, range(3, loads))
        scatter_pack(c)
        scatter_send(c - 2, rows(c - 2, 2 * H, STRIDE - 1 - 2 * H))

    def reduce(c, first=False):
        unpack_high(SCATTER_IN, c, first=first)
        origin_in = origin_of(SCATTER_IN)
        origin = None if first else origin_of(OWN)
        high = []
        for g in range(GROUPS):
            if g == 2:
                send(OWN, FROM_Y, rows(c, 0, 2 * H), sem(FROM_Y, c), ypeer).start()
                wait(SCATTER_IN, rows(c, 0, 2 * H), late_sem.at[c])
            sums = []
            for k, theirs in zip((2 * g, 2 * g + 1), unpack_low(SCATTER_IN, c, g, g ^ 2, origin_in)):
                total = (tile(1, c, k) + theirs.astype(jnp.float32)).astype(jnp.bfloat16)
                put(mx, my, c, k, total)
                sums.append(pltpu.bitcast(total, I32))
            if origin is None:
                origin = _pick_origin(sums[0])
                msg[OWN, pl.ds(0, 8), :] = origin[:8]
            high.append(pack_low(OWN, c, g, *sums, origin))
        pack_signs(OWN, c, high)
        send(OWN, FROM_Y, rows(c, 2 * H, CODE - 2 * H), sem(FROM_Y, c), ypeer).start()
        pack_high(OWN, c, high, [(FROM_Y, ypeer), (FROM_X, xpeer)])
        send(OWN, FROM_Y, code_rows(c, H - 1), sem(FROM_Y, c), ypeer, rows(c, CODE, H - 1)).start()

    def store(s, c, keep=0):
        qx = jnp.where(s == FROM_Y, mx, 1 - mx)
        qy = jnp.where(s == FROM_X, my, 1 - my)
        origin = origin_of(s)
        for g in range(GROUPS):
            for k, value in zip((2 * g, 2 * g + 1), unpack_low(s, c, g, g, origin, keep)):
                put(qx, qy, c, k, value)

    tail = CHUNKS - TAIL
    via_y = [(rows(tail, 0, SIGN), sem(FROM_D, tail)),
             (rows(tail + 1, 0, VIA_Y), sem(FROM_D, tail + 1))]
    small_via_x = [(rows(c, SIGN, H // 2),) * 2 for c in range(tail, CHUNKS)] + [
        (rows(LAST, CODE, H - 1), code_rows(LAST, H - 1)), (rows(CHUNKS, CODE, H), code_rows(CHUNKS, H))]
    low_via_x = [(pl.ds(BASE + (tail + 1) * STRIDE + VIA_Y, SIGN - VIA_Y), edge_sem.at[0]),
                 (rows(LAST, 0, SIGN), sem(FROM_D, LAST))]

    def step(i, _):
        @pl.when(i <= LAST)
        def _():
            wait_load(1, i, range(1, loads))
            pl.when(i < LAST - 1)(
                lambda: wait(SCATTER_IN, rows(i, 2 * H, STRIDE - 1 - 2 * H), sem(SCATTER_IN, i)))
            for c in (LAST - 1, LAST):
                pl.when(i == c)(lambda: wait(SCATTER_IN, chunk_rows(c, 2 * H), sem(SCATTER_IN, c)))
            reduce(i)

            def to_x(part):
                front, back = halves(part)
                send(OWN, FROM_X, front, sem(FROM_X, i - 2), xpeer).start()
                send(OWN, FROM_X, back, late_sem.at[CHUNKS + i - 2], xpeer).start()

            inner_chunk(i - 2, to_x)

            @pl.when(i == LAST)
            def _():
                flush(OWN)
                send(OWN, FROM_Y, code_rows(CHUNKS, H), edge_sem.at[1], ypeer, rows(CHUNKS, CODE, H)).start()
                for c in (LAST - 1, LAST):
                    send(OWN, FROM_X, chunk_rows(c), sem(FROM_X, c), xpeer).start()

        pl.when(i + AHEAD + 2 <= LAST)(lambda: scatter(i + AHEAD + 2))
        pl.when(i + AHEAD + 2 == CHUNKS)(lambda: flush(SCATTER_OUT))
        for c in (LAST - 1, LAST):
            pl.when(i + AHEAD == c)(lambda: scatter_send(c, chunk_rows(c, 2 * H)))

        f = i - AHEAD - 1

        def relay(part):
            for half, arrived in zip(halves(part), (sem(FROM_X, f), late_sem.at[CHUNKS + f])):
                wait(FROM_X, half, arrived)
                pl.when(f < tail)(lambda: send(FROM_X, FROM_D, half, sem(FROM_D, f), ypeer).start())

        inner_chunk(f, relay)
        for c in (LAST - 1, LAST):
            pl.when(f == c)(lambda: wait(FROM_X, chunk_rows(c), sem(FROM_X, c)))
        for c, (part, arrived) in enumerate(via_y, tail):
            pl.when(f == c)(lambda: send(FROM_X, FROM_D, part, arrived, ypeer).start())

        g = i - 2
        pl.when(g == 0)(lambda: wait(FROM_Y, pl.ds(BASE - 1, STRIDE), sem(FROM_Y, 0)))
        pl.when(jnp.logical_and(g > 0, g <= LAST))(
            lambda: wait(FROM_Y, rows(g, 0, STRIDE - 1), sem(FROM_Y, g)))

        @pl.when(g == LAST)
        def _():
            wait(FROM_Y, rows(CHUNKS, CODE, H), edge_sem.at[1])
            for k, (part, dst_part) in enumerate(small_via_x):
                send(FROM_Y, FROM_D, part, edge_sem.at[5 + k], xpeer, dst_part).start()
            for part, arrived in low_via_x:
                send(FROM_Y, FROM_D, part, arrived, xpeer).start()

        from_y = jnp.where(g < LAST, 1, jnp.where(g == LAST, 3, 0))

        def gather(j, _):
            s = jnp.where(j == 0, FROM_X, jnp.where(j <= from_y, FROM_Y, FROM_D))
            c = jnp.where(j == 0, f, jnp.where(j <= from_y, g - 3 + j, f - 2))

            @pl.when(c >= 0)
            def _():
                pl.when(s == FROM_D)(
                    lambda: inner_chunk(c, lambda part: wait(FROM_D, part, sem(FROM_D, c))))
                unpack_high(s, c)
                store(s, c)

        lax.fori_loop(0, 1 + from_y + (f - 2 < tail), gather, None)

    def first_send(part, arrived):
        send(SCATTER_OUT, SCATTER_IN, part, arrived, xpeer).start()

    first_words = [pl.ds(ORIGIN, H), code_rows(1, H - 1), code_rows(2, H - 1)]
    first_tiles.wait()
    high0, origin0 = scatter_group(0, 0, None)
    pl.when(is_00)(lambda: pl.semaphore_wait(barrier, 2))
    pl.when(jnp.logical_not(is_00))(lambda: pl.semaphore_wait(barrier, 1))
    first_send(rows(0, 2 * H, H), sem(SCATTER_IN, 0))
    pl.when(is_00)(lambda: notify(hello_sem, ypeer))
    other_tiles.wait()
    high0 = [high0] + [scatter_group(0, g, origin0)[0] for g in range(1, GROUPS)]
    pack_signs(SCATTER_OUT, 0, high0)
    first_send(rows(0, 3 * H, CODE - 3 * H), sem(SCATTER_IN, 0))
    pack_high(SCATTER_OUT, 0, high0, [(SCATTER_IN, xpeer)])
    first_send(first_words[0], edge_sem.at[2])

    @pl.when(is_01)
    def _():
        pl.semaphore_wait(hello_sem, 1)
        notify(hello_sem, xpeer)
        notify(hello_sem, ypeer)

    for c in (1, 2):
        load(0, c).wait()
        scatter_pack(c)
        first_send(first_words[c], edge_sem.at[2 + c])
        if c == 1:
            first_send(rows(0, 0, 2 * H), late_sem.at[0])
    lax.fori_loop(3, AHEAD + 2, scatter, None)
    pl.when(jnp.logical_not(is_01))(lambda: pl.semaphore_wait(hello_sem, 1))
    pl.when(is_00)(lambda: notify(hello_sem, xpeer))

    load(1, 0).wait()
    wait(SCATTER_IN, rows(0, 2 * H, CODE - 2 * H), sem(SCATTER_IN, 0))
    wait(SCATTER_IN, first_words[0], edge_sem.at[2])
    wait(SCATTER_IN, first_words[1], edge_sem.at[3])
    reduce(0, first=True)
    send(OWN, FROM_Y, pl.ds(ORIGIN, 1), sem(FROM_Y, 0), ypeer, pl.ds(BASE - 1, 1)).start()
    wait(SCATTER_IN, first_words[2], edge_sem.at[4])
    state[SCATTER_IN, 1] = _unfold_rows(msg[SCATTER_IN, code_rows(2, H), :])
    scatter(AHEAD + 2)

    lax.fori_loop(1, CHUNKS + AHEAD + 1, step, None)

    for k, (_, dst_part) in enumerate(small_via_x):
        wait(FROM_D, dst_part, edge_sem.at[5 + k])
    lax.fori_loop(0, TAIL, lambda j, _: unpack_high(FROM_D, tail + j, j), None)

    def finish(j, _):
        for k, (part, arrived) in zip((0, 1, 1, 2), via_y + low_via_x):
            pl.when(j == k)(lambda: wait(FROM_D, part, arrived))
        store(FROM_D, tail + j, j)

    lax.fori_loop(0, TAIL, finish, None)

    sent = msg.at[pl.ds(0, 4), pl.ds(0, 1 + CHUNKS * (STRIDE - 1) + H + 1)]
    pltpu.make_async_copy(sent, sent, send_sem).wait()
    lax.fori_loop(
        0, raw_sends[0], lambda j, _: send_raw(SCATTER_OUT, SCATTER_IN, 0, xpeer).wait_send(), None)


def pallas_dist_rsx_agy_m2048_n1024_kernel(x: jax.Array):
    dma = pltpu.SemaphoreType.DMA
    return pl.pallas_call(
        _body,
        out_shape=jax.ShapeDtypeStruct((M, 2 * N), jnp.bfloat16),
        in_specs=[pl.BlockSpec(memory_space=pltpu.HBM)],
        out_specs=pl.BlockSpec(memory_space=pltpu.VMEM),
        scratch_shapes=[
            pltpu.VMEM((2, HALF, N), jnp.float32),
            pltpu.VMEM((6, BASE + (CHUNKS + 1) * STRIDE, LANES), I32),
            pltpu.VMEM((6, CHUNKS * GROUPS * H, LANES), I32),
            pltpu.VMEM((6, 4, H, LANES), I32),
            pltpu.VMEM((TAIL, GROUPS, H, LANES), I32),
            pltpu.SMEM((1,), I32),
            dma((13,)),
            dma((4 * CHUNKS,)),
            dma((2 * CHUNKS,)),
            dma((4 * CHUNKS,)),
            dma((10,)),
            dma,
            dma,
            pltpu.SemaphoreType.REGULAR,
        ],
        compiler_params=pltpu.CompilerParams(
            collective_id=0,
            vmem_limit_bytes=64 * 2**20,
            disable_semaphore_checks=True,
        ),
        name="rsx_agy",
    )(x)
```
